```python
import numpy as np

kernel_name = "dist_pipemlp_pp2tp2_xy_b4096_d256_h512"

def setup_inputs():
    x_padded = np.zeros((2, 4096, 256), dtype=np.float32)
    x_padded[0] = np.random.randn(4096, 256).astype(np.float32)
    Win = np.random.randn(4, 256, 1024).astype(np.float32)
    Wout = np.random.randn(4, 1024, 256).astype(np.float32)
    return {"x_padded": x_padded, "Win": Win, "Wout": Wout}

def reference(x_padded, Win, Wout):
    a = x_padded[0]
    for k in range(4):
        h = a @ Win[k]
        h = np.maximum(h, 0.0)
        a = h @ Wout[k]
    out = np.zeros_like(x_padded)
    out[1] = a
    return out
```

```python
import contextlib

import jax
import jax.numpy as jnp
from jax import lax
from jax.experimental import pallas as pl
from jax.experimental.pallas import tpu as pltpu

_BF16 = jnp.bfloat16
_F32 = jnp.float32

_CONFIG = dict(
    chunks=(128,) * 16,
    parts=(1,) * 16,
    l2_rows=(0,) * 8 + (80,) * 8,
    early=5,
    early_h=1,
    merged=((1, 2), (3, 4)),
    twin=(0,),
    detour=(6, 8, 10),
    detour_rows=None,
    detour_at=(12, 14, 15),
    drain={9: (1, 2), 11: (3, 4), 13: (5, 7)},
    win_pieces=((0, 16), (16, 48), (64, 192)),
    wout_pieces=((0, 512),),
    first_loads=2,
    l0_rows=512,
    own_first=1024,
    own_gap_rows=128,
    x_ahead=2,
    roll=True,
    scopes=False,
)


def _make_kernel(cfg, rows, d, hid):
    half = rows // 2
    chunks, parts = tuple(cfg["chunks"]), tuple(cfg["parts"])
    assert sum(chunks) == half and len(parts) == len(chunks)
    n, n_parts = len(chunks), sum(parts)
    row0 = [sum(chunks[:i]) for i in range(n)]
    part0 = [sum(parts[:i]) for i in range(n)]
    l2_rows = tuple(cfg["l2_rows"])
    first_l2 = [i for i in range(n) if l2_rows[i]][:1]
    early, early_h, twin = cfg["early"], cfg["early_h"], tuple(cfg["twin"])
    merged = {g[0]: tuple(g) for g in cfg["merged"]}
    batches, i = [], 0
    while i < n:
        batches.append(merged.get(i, (i,)))
        i = batches[-1][-1] + 1
    detour, detour_at = tuple(cfg["detour"]), tuple(cfg["detour_at"])
    detour_rows = tuple(cfg["detour_rows"] or [chunks[i] for i in detour])
    n_arrived = cfg.get("tail_arrived", 0)
    assert twin == tuple(range(len(twin))) and len(twin) <= early
    assert not any(i in twin for i in detour)
    drain = {i: tuple(v) for i, v in cfg["drain"].items()}
    drained = [j for i in sorted(drain) for j in drain[i]]
    assert not any(j in detour or j in twin for j in drained)
    tail = cfg.get("tail")
    if tail is None:
        tail = [j for j in range(n) if j not in drained and j not in twin and j not in detour]
        tail = tail[:-1] + list(detour) + tail[-1:]
    assert sorted(drained + list(tail) + list(twin)) == list(range(n))
    w_pieces = ([(0, r, m) for r, m in cfg["win_pieces"]]
                + [(1, r, m) for r, m in cfg["wout_pieces"]])
    n_wp, n_win, first_loads = len(w_pieces), len(cfg["win_pieces"]), cfg["first_loads"]
    l0_rows, x_ahead = cfg["l0_rows"], cfg["x_ahead"]
    own_first, gap_rows = cfg["own_first"], cfg["own_gap_rows"]
    n_l0 = (half + own_first) // l0_rows
    n_gap = (half - own_first) // gap_rows
    assert all(own_first + i * gap_rows >= row0[i] + chunks[i] for i in range(n_gap))

    def layout(*groups):
        base, at = {}, 0
        for name, count in groups:
            base[name] = at
            at += count
        return base, at

    common = (("tx", 1), ("w_ld", 2 * n_wp), ("w", 4))
    main0, n_main0 = layout(*common, ("partial", n_parts), ("x_ld", n_l0 + 1), ("l2", 2),
                            ("hop", len(detour)))
    main1, n_main1 = layout(*common, ("act", n), ("twin", len(twin)), ("out", len(drained)))
    n_last = 1 + max(len(detour), len(tail))

    def scope(name):
        return jax.named_scope(name) if cfg["scopes"] else contextlib.nullcontext()

    def rows_at(r, m):
        return pl.ds(r if isinstance(r, int) else pl.multiple_of(r, 16), m)

    def for_chunks(idx, signature, body):
        idx = list(idx)
        p = 0
        while p < len(idx):
            i0, q = idx[p], p + 1
            while (cfg["roll"] and q < len(idx) and idx[q] == i0 + q - p
                   and (chunks[idx[q]], parts[idx[q]]) == (chunks[i0], parts[i0])
                   and signature(idx[q]) is not None
                   and signature(idx[q]) == signature(i0)):
                q += 1
            if q - p == 1:
                body(i0, 0)
            else:
                def step(k, carry, i0=i0):
                    body(i0, k)
                    return carry
                lax.fori_loop(0, q - p, step, 0)
            p = q

    def runs(batch, key):
        res = []
        for i in batch:
            if res and key(res[-1][0]) == key(i):
                res[-1] = (res[-1][0], res[-1][1] + chunks[i])
            else:
                res.append((i, chunks[i]))
        return res

    def hidden(a, wi):
        h = jnp.dot(a, wi[...], preferred_element_type=_F32)
        return jnp.maximum(h, 0.0).astype(_BF16)

    def half_layer(a, wi, wo):
        return jnp.dot(hidden(a, wi), wo[...], preferred_element_type=_F32)

    def chunk_rows(i0, k=0):
        return rows_at(row0[i0] + k * chunks[i0], chunks[i0])

    def chunk_parts(i0, k=0):
        m = chunks[i0] // parts[i0]
        return [(part0[i0] + k * parts[i0] + j,
                 rows_at(row0[i0] + k * chunks[i0] + j * m, m))
                for j in range(parts[i0])]

    def kernel(
        x_hbm, win_hbm, wout_hbm, out_ref,
        wi_f32, wo_f32, wi_own, wo_own, wi_nbr, wo_nbr, wi_l2, wo_l2,
        x_buf, acc, h_buf, p_send, p_recv, a_send, a_recv, o_send, o_recv, last_sems,
    ):
        mx, my = lax.axis_index("x"), lax.axis_index("y")
        y_nbr, x_nbr = (mx, 1 - my), (1 - mx, my)
        own0 = pl.multiple_of(my * half, half)
        oth0 = pl.multiple_of((1 - my) * half, half)
        w_hbm, w_f32 = (win_hbm, wout_hbm), (wi_f32, wo_f32)
        w_own, w_nbr, w_l2 = (wi_own, wo_own), (wi_nbr, wo_nbr), (wi_l2, wo_l2)
        last_tx = last_sems.at[0]

        def remote(src, dst, tx, rx, dev):
            return pltpu.make_async_remote_copy(
                src, dst, tx, rx, device_id=dev, device_id_type=pl.DeviceIdType.MESH)

        def signal(sem, dev):
            pl.semaphore_signal(
                sem, inc=1, device_id=dev, device_id_type=pl.DeviceIdType.MESH)

        def full_layer(a, l):
            return (half_layer(a, wi_own.at[l], wo_own.at[l])
                    + half_layer(a, wi_nbr.at[l], wo_nbr.at[l]))

        def write_out(col0, i0, k, val):
            r = col0 + row0[i0] + k * chunks[i0]
            out_ref[0, rows_at(r, chunks[i0]), :] = val.astype(_F32)

        def finish_early(batch):
            h = [hidden(a_send[pl.ds(row0[i], m), :], wi_nbr.at[1]) if i < early_h
                 else h_buf[pl.ds(row0[i], m), :]
                 for i, m in runs(batch, lambda i: i < early_h)]
            sl = pl.ds(row0[batch[0]], sum(chunks[i] for i in batch))
            return acc[sl, :] + jnp.dot(jnp.concatenate(h), wo_nbr[1], preferred_element_type=_F32)

        def detour_part(i):
            return pl.ds(row0[i], detour_rows[detour.index(i)])

        def tail_copy(i, skip=0):
            sl = pl.ds(row0[i] + skip, chunks[i] - skip)
            return remote(o_send.at[sl], o_recv.at[sl], last_tx,
                          last_sems.at[1 + tail.index(i)], y_nbr)

        def second_hop(i):
            sl = detour_part(i)
            return remote(o_send.at[sl], o_recv.at[sl], last_tx,
                          last_sems.at[1 + detour.index(i)], y_nbr)

        def third_hop(i):
            sl = detour_part(i)
            return remote(o_recv.at[sl], o_recv.at[sl], last_tx,
                          last_sems.at[1 + tail.index(i)], x_nbr)

        def main_phase(sems, x_ready):
            barrier = pltpu.get_barrier_semaphore()
            tx = sems.at[main0["tx"]]

            def load_piece(l, j):
                k, r, m = w_pieces[j]
                return pltpu.make_async_copy(
                    w_hbm[k].at[l, pl.ds(r, m)], w_f32[k].at[l, pl.ds(r, m)],
                    sems.at[main0["w_ld"] + l * n_wp + j])

            def cast_piece(l, j):
                k, r, m = w_pieces[j]
                w_own[k][l, pl.ds(r, m), :] = w_f32[k][l, pl.ds(r, m), :].astype(_BF16)

            def send_piece(l, j):
                k, r, m = w_pieces[j]
                remote(w_own[k].at[l, pl.ds(r, m)], w_nbr[k].at[l, pl.ds(r, m)],
                       tx, sems.at[main0["w"] + 2 * l + k], y_nbr).start()

            def swap_pieces(l, js):
                for j in js:
                    load_piece(l, j).wait()
                    cast_piece(l, j)
                    send_piece(l, j)

            def swap_first_win(l, n_signals, start_next_loads):
                load_piece(l, 0).wait()
                for j in range(first_loads, n_win):
                    load_piece(l, j).start()
                cast_piece(l, 0)
                with scope("s0_barrier"):
                    pl.semaphore_wait(barrier, n_signals)
                send_piece(l, 0)
                swap_pieces(l, range(1, n_win - 1))
                load_piece(l, n_win - 1).wait()
                start_next_loads()
                cast_piece(l, n_win - 1)
                send_piece(l, n_win - 1)

            def weight_swap(l, k):
                return remote(w_own[k].at[l], w_nbr[k].at[l],
                              tx, sems.at[main0["w"] + 2 * l + k], y_nbr)

            def l2_copy(s, k):
                return remote((w_own, w_nbr)[s][k].at[0], w_l2[k].at[s],
                              tx, sems.at[main0["l2"] + k], x_nbr)

            def l2_both(k):
                return remote(w_l2[k], w_l2[k], tx, sems.at[main0["l2"] + k], x_nbr)

            def partial_copy(j, sl):
                return remote(p_send.at[sl], p_recv.at[sl], tx,
                              sems.at[main0["partial"] + j], y_nbr)

            def act_copy(i, sl):
                return remote(a_send.at[sl], a_recv.at[sl], last_tx,
                              sems.at[main1["act"] + i], x_nbr)

            def twin_copy(i):
                sl = chunk_rows(i)
                return remote(a_send.at[sl], p_recv.at[sl], tx,
                              sems.at[main1["twin"] + twin.index(i)], y_nbr)

            def drained_copy(i):
                sl = chunk_rows(i)
                return remote(o_send.at[sl], o_recv.at[sl], last_tx,
                              sems.at[main1["out"] + drained.index(i)], y_nbr)

            def first_hop(i):
                sl = detour_part(i)
                return remote(o_send.at[sl], o_send.at[sl], last_tx,
                              sems.at[main0["hop"] + detour.index(i)], x_nbr)

            @pl.when(mx == 0)
            def stage0():
                def x_load(j, r, m):
                    src0 = pl.multiple_of((oth0 + r) % rows, 16)
                    return pltpu.make_async_copy(
                        x_hbm.at[0, pl.ds(src0, m)], x_buf.at[rows_at(r, m)],
                        sems.at[main0["x_ld"] + j])

                def x_block(j):
                    return x_load(j, j * l0_rows, l0_rows)

                def x_rest():
                    return x_load(n_l0, half + own_first, half - own_first)

                def start_layer0_loads():
                    for j in range(n_wp):
                        load_piece(0, j).start()
                    x_block(0).start()

                for j in range(first_loads):
                    load_piece(1, j).start()
                signal(barrier, y_nbr)
                signal(barrier, x_nbr)
                with scope("s0_w1"):
                    swap_first_win(1, 1, start_layer0_loads)
                with scope("s0_w0"):
                    for j in range(n_wp):
                        load_piece(0, j).wait()
                        cast_piece(0, j)
                    for j in range(1, x_ahead):
                        x_block(j).start()
                    for j in range(n_win, n_wp):
                        load_piece(1, j).start()

                def layer0(sl):
                    return half_layer(x_buf[sl, :].astype(_BF16), wi_own.at[0], wo_own.at[0])

                def layer0_block(j):
                    x_block(j).wait()

                    @pl.when(j + x_ahead < n_l0)
                    def _():
                        x_block(j + x_ahead).start()

                    return layer0(rows_at(j * l0_rows, l0_rows))

                with scope("s0_l0_oth"):
                    def l0_other(j, carry):
                        p_send[rows_at(j * l0_rows, l0_rows), :] = layer0_block(j).astype(_BF16)
                        pl.when(j == 0)(lambda: swap_pieces(1, range(n_win, n_wp)))
                        return carry
                    lax.fori_loop(0, half // l0_rows, l0_other, 0)
                if n_gap:
                    x_rest().start()
                with scope("s0_l0_own"):
                    all_parts = [part for i in range(n) for part in chunk_parts(i)]
                    n_own = own_first // l0_rows
                    for b in range(n_own):
                        j = half // l0_rows + b
                        x_block(j).wait()
                        if j + x_ahead < n_l0:
                            x_block(j + x_ahead).start()
                        for q, sl in all_parts[b * n_parts // n_own:(b + 1) * n_parts // n_own]:
                            partial_copy(q, sl).start()
                        acc[pl.ds(b * l0_rows, l0_rows), :] = layer0(pl.ds(j * l0_rows, l0_rows))

                with scope("s0_wait_w1"):
                    if n_gap:
                        x_rest().wait()
                    pl.semaphore_wait(x_ready, 1)
                    for k in range(2):
                        weight_swap(1, k).wait_recv()

                def signature(i):
                    if i in first_l2 or i in detour_at:
                        return None
                    return (l2_rows[i], i < n_gap)

                def stream(i0, k):
                    for p, (j, sl) in enumerate(chunk_parts(i0, k)):
                        with scope("s0_wait_p"):
                            partial_copy(j, sl).wait_recv()
                        with scope("s0_l1"):
                            a = (acc[sl, :] + p_recv[sl, :].astype(_F32)).astype(_BF16)
                            a = full_layer(a, 1).astype(_BF16)
                            m = chunks[i0] // parts[i0]
                            r = row0[i0] + k * chunks[i0] + p * m
                            plain = min(max(chunks[i0] - l2_rows[i0] - p * m, 0), m)
                            if plain:
                                a_send[rows_at(r, plain), :] = a[:plain]
                                act_copy(i0 + k, rows_at(r, plain)).start()
                            if plain < m:
                                if i0 in first_l2 and p == (chunks[i0] - l2_rows[i0]) // m:
                                    for w in range(2):
                                        l2_both(w).wait_recv()
                                a = a[plain:]
                                a = (half_layer(a, wi_l2.at[0], wo_l2.at[0])
                                     + half_layer(a, wi_l2.at[1], wo_l2.at[1])).astype(_BF16)
                                a_send[rows_at(r + plain, m - plain), :] = a
                                act_copy(i0 + k, rows_at(r + plain, m - plain)).start()
                    m = 2 * chunks[i0]
                    out_ref[0, rows_at(2 * row0[i0] + k * m, m), :] = jnp.zeros((m, d), _F32)
                    if i0 < n_gap:
                        r = own_first + (i0 + k) * gap_rows
                        acc[rows_at(r, gap_rows), :] = layer0(rows_at(half + r, gap_rows))
                    for i, at in zip(detour, detour_at):
                        if at == i0:
                            with scope("s0_wait_d0"):
                                first_hop(i).wait_recv()
                            second_hop(i).start()

                for_chunks(range(n), signature, stream)
                for k in range(2):
                    weight_swap(1, k).wait_send()
                partial_copy(0, pl.ds(0, half)).wait_send()

            @pl.when(mx == 1)
            def stage1():
                def start_other_loads():
                    for j in range(n_win, n_wp):
                        load_piece(0, j).start()
                    for j in range(n_wp):
                        load_piece(1, j).start()

                for j in range(first_loads):
                    load_piece(0, j).start()
                signal(barrier, y_nbr)
                with scope("s1_w"):
                    swap_first_win(0, 2, start_other_loads)
                    signal(x_ready, x_nbr)
                    if first_l2:
                        l2_copy(0, 0).start()
                    swap_pieces(0, range(n_win, n_wp))
                    if first_l2:
                        l2_copy(0, 1).start()
                    swap_pieces(1, range(n_wp))
                with scope("s1_wait_w2"):
                    for k in range(2):
                        weight_swap(0, k).wait_recv()
                        if first_l2:
                            l2_copy(1, k).start()

                def wait_act(i0, k):
                    with scope("s1_wait_a"):
                        act_copy(i0 + k, chunk_rows(i0, k)).wait_recv()

                def layer2(batch, k=0):
                    todo, done = [], []
                    for i in batch:
                        r, plain = row0[i] + k * chunks[i], chunks[i] - l2_rows[i]
                        if plain:
                            todo.append(a_recv[rows_at(r, plain), :])
                        done.append((plain, a_recv[rows_at(r + plain, l2_rows[i]), :]
                                     if l2_rows[i] else None))
                    if todo:
                        todo = full_layer(jnp.concatenate(todo), 0).astype(_BF16)
                    res, r = [], 0
                    for plain, rest in done:
                        if plain:
                            res.append(todo[r:r + plain])
                            r += plain
                        if rest is not None:
                            res.append(rest)
                    return jnp.concatenate(res)

                def wait_drained(i0):
                    for i in drain.get(i0, ()):
                        with scope("s1_wait_o"):
                            drained_copy(i).wait_recv()

                def emit(i, out):
                    out = out.astype(_BF16)
                    o_send[chunk_rows(i), :] = out
                    write_out(own0, i, 0, out)
                    for j in drain.get(i, ()):
                        write_out(oth0, j, 0, o_recv[chunk_rows(j), :])
                    if i in detour:
                        first_hop(i).start()
                        skip = detour_rows[detour.index(i)]
                        if skip < chunks[i]:
                            tail_copy(i, skip).start()
                    else:
                        (drained_copy if i in drained else tail_copy)(i).start()

                def early_own(i0, k):
                    sl = chunk_rows(i0, k)
                    wait_act(i0, k)
                    a = layer2((i0,), k)
                    if i0 in twin or i0 < early_h:
                        a_send[sl, :] = a
                    if i0 in twin:
                        twin_copy(i0).start()
                    acc[sl, :] = half_layer(a, wi_own.at[1], wo_own.at[1])
                    if i0 >= early_h:
                        h_buf[sl, :] = hidden(a, wi_nbr.at[1])

                def signature(i):
                    return None if i in twin else (l2_rows[i],)

                for_chunks(range(min(early, early_h)), signature, early_own)
                with scope("s1_wait_w3"):
                    weight_swap(1, 0).wait_recv()
                for_chunks(range(early_h, early), signature, early_own)
                with scope("s1_wait_w3"):
                    weight_swap(1, 1).wait_recv()
                for batch in batches:
                    if batch[0] in twin:
                        continue
                    for i in batch:
                        wait_drained(i)
                    if batch[0] < early:
                        out = finish_early(batch)
                    else:
                        for i in batch:
                            wait_act(i, 0)
                        out = full_layer(layer2(batch), 1)
                    for i in batch:
                        r = row0[i] - row0[batch[0]]
                        emit(i, out[r:r + chunks[i]])
                for s in range(4):
                    weight_swap(s // 2, s % 2).wait_send()
                    if first_l2:
                        l2_copy(s // 2, s % 2).wait_send()
                for i in twin:
                    twin_copy(i).wait()

        pl.run_scoped(main_phase, pltpu.SemaphoreType.DMA((max(n_main0, n_main1),)),
                      pltpu.SemaphoreType.REGULAR)

        @pl.when(mx == 0)
        def finish0():
            for i in detour:
                with scope("s0_wait_d1"):
                    second_hop(i).wait_recv()
                third_hop(i).start()
            with scope("s0_fin"):
                remote(a_send, a_recv, last_tx, last_tx, x_nbr).wait_send()
                for i in detour:
                    second_hop(i).wait_send()
                    third_hop(i).wait_send()

        @pl.when(mx == 1)
        def finish1():
            with scope("s1_twin"):
                for i in tail[:n_arrived]:
                    tail_copy(i).wait_recv()
                if twin:
                    m = sum(chunks[i] for i in twin)
                    for col0, out in ((own0, finish_early(twin)),
                                      (oth0, full_layer(p_recv[pl.ds(0, m), :], 1))):
                        out_ref[0, rows_at(col0, m), :] = out.astype(_BF16).astype(_F32)
                for i in tail[:n_arrived]:
                    write_out(oth0, i, 0, o_recv[chunk_rows(i), :])
            for i in tail[n_arrived:]:
                if i == tail[-1]:
                    sl = pl.ds(row0[len(twin)], half - row0[len(twin)])
                    remote(o_send.at[sl], o_recv.at[sl], last_tx, last_tx, y_nbr).wait_send()
                with scope("s1_wait_o"):
                    tail_copy(i).wait_recv()
                write_out(oth0, i, 0, o_recv[chunk_rows(i), :])

    scratch = [
        pltpu.VMEM((2, d, hid), _F32), pltpu.VMEM((2, hid, d), _F32),
        *[pltpu.VMEM(shape, _BF16) for _ in range(3) for shape in ((2, d, hid), (2, hid, d))],
        pltpu.VMEM((rows, d), _F32), pltpu.VMEM((half, d), _F32),
        pltpu.VMEM((row0[early], hid), _BF16),
        *[pltpu.VMEM((half, d), _BF16) for _ in range(6)],
        pltpu.SemaphoreType.DMA((n_last,)),
    ]
    return kernel, scratch


def _run(cfg, x_padded, Win, Wout):
    _, rows, d = x_padded.shape
    kernel, scratch = _make_kernel(cfg, rows, d, Win.shape[2])
    hbm = pl.BlockSpec(memory_space=pltpu.HBM)
    return pl.pallas_call(
        kernel,
        out_shape=pltpu.VMEM(x_padded.shape, x_padded.dtype),
        in_specs=[hbm, hbm, hbm],
        out_specs=pl.BlockSpec(memory_space=pltpu.VMEM),
        scratch_shapes=scratch,
        compiler_params=pltpu.CompilerParams(
            collective_id=0, vmem_limit_bytes=64 * 1024 * 1024, **cfg.get("params", {})),
    )(x_padded, Win, Wout)


def pallas_dist_pipemlp_pp2tp2_xy_b4096_d256_h512_kernel(
    x_padded: jax.Array,
    Win: jax.Array,
    Wout: jax.Array,
):
    return _run(_CONFIG, x_padded, Win, Wout)
```

```python
import functools

import jax
import jax.numpy as jnp
from jax import lax
from jax.experimental import pallas as pl
from jax.experimental.pallas import tpu as pltpu

_BF16 = jnp.bfloat16
_F32 = jnp.float32

_ROWS, _D, _HID = 4096, 256, 512
_HALF = _ROWS // 2
_C = 128
_N = _HALF // _C

_L2_PLAN = ((0, 8, 0), (8, 9, 80), (9, 12, 80), (12, 16, 64))
_TWIN, _EARLY = 2, 6
_EARLY_BATCH = 2
_DETOUR = {6: 12, 8: 14, 10: 15}
_DRAIN = {9: 2, 10: 3, 11: 4, 12: 5, 13: 7, 14: 9}
_TAIL = (11, 12, 6, 13, 8, 14, 10, 15)
_TAIL_ARRIVED = 3
assert sorted((*range(_TWIN), *_DRAIN.values(), *_TAIL)) == list(range(_N))
assert set(_DETOUR) <= set(_TAIL[:-1])

_W_PIECES = ((0, 0, 16), (0, 16, 48), (0, 64, 192), (1, 0, 512))
_N_WP, _N_WIN = len(_W_PIECES), 3
_L0_ROWS = 512
_N_GAP = 8
_N_L0 = (_ROWS - _N_GAP * _C) // _L0_ROWS


def _layout(*groups):
    base, at = {}, 0
    for name, count in groups:
        base[name] = at
        at += count
    return base, at


_BOTH = (("tx", 1), ("w_load", 2 * _N_WP), ("w", 4))
_SEM0, _N_SEM0 = _layout(*_BOTH, ("x_load", _N_L0 + 1), ("partial", _N), ("l2", 2),
                         ("detour", len(_DETOUR)))
_SEM1, _N_SEM1 = _layout(*_BOTH, ("act", _N), ("twin", _TWIN), ("drain", len(_DRAIN)))


def _rows(r, m=_C):
    return pl.ds(r if isinstance(r, int) else pl.multiple_of(r, 16), m)


def _chunk(i, count=1):
    return _rows(i * _C, count * _C)


def _loop(lo, hi, body):
    if hi - lo == 1:
        body(lo)
    else:
        def step(i, carry):
            body(i)
            return carry
        lax.fori_loop(lo, hi, step, 0)


def _hidden(a, wi):
    h = jnp.dot(a, wi[...], preferred_element_type=_F32)
    return jnp.maximum(h, 0.0).astype(_BF16)


def _half_layer(a, wi, wo):
    return jnp.dot(_hidden(a, wi), wo[...], preferred_element_type=_F32)


def _kernel(
    x_hbm, win_hbm, wout_hbm, out_ref,
    wi_f32, wo_f32, wi_own, wo_own, wi_nbr, wo_nbr, wi_l2, wo_l2,
    x_buf, acc, h_buf, p_send, p_recv, a_send, a_recv, o_send, o_recv, last_tx, last_rx,
):
    mx, my = lax.axis_index("x"), lax.axis_index("y")
    y_nbr, x_nbr = (mx, 1 - my), (1 - mx, my)
    own0, oth0 = my * _HALF, (1 - my) * _HALF
    w_hbm, w_f32 = (win_hbm, wout_hbm), (wi_f32, wo_f32)
    w_own, w_nbr, w_l2 = (wi_own, wo_own), (wi_nbr, wo_nbr), (wi_l2, wo_l2)
    detours = list(_DETOUR)

    def remote(src, dst, tx, rx, dev):
        return pltpu.make_async_remote_copy(
            src, dst, tx, rx, device_id=dev, device_id_type=pl.DeviceIdType.MESH)

    def signal(sem, dev):
        pl.semaphore_signal(sem, inc=1, device_id=dev, device_id_type=pl.DeviceIdType.MESH)

    def full_layer(a, l):
        return (_half_layer(a, wi_own.at[l], wo_own.at[l])
                + _half_layer(a, wi_nbr.at[l], wo_nbr.at[l]))

    def write_received(j):
        out_ref[0, _rows(oth0 + j * _C), :] = o_recv[_chunk(j), :].astype(_F32)

    def tail_sem(end_sems, j):
        return last_rx if j == _TAIL[-1] else end_sems.at[_TAIL.index(j)]

    def tail_copy(end_sems, j):
        return remote(o_send.at[_chunk(j)], o_recv.at[_chunk(j)], last_tx,
                      tail_sem(end_sems, j), y_nbr)

    def second_hop(end_sems, j):
        return remote(o_send.at[_chunk(j)], o_recv.at[_chunk(j)], last_tx,
                      end_sems.at[detours.index(j)], y_nbr)

    def third_hop(end_sems, j):
        return remote(o_recv.at[_chunk(j)], o_recv.at[_chunk(j)], last_tx,
                      tail_sem(end_sems, j), x_nbr)

    def main_phase(end_sems, sems, x_ready):
        barrier = pltpu.get_barrier_semaphore()
        tx = sems.at[_SEM0["tx"]]

        def load_piece(l, j):
            k, r, m = _W_PIECES[j]
            return pltpu.make_async_copy(
                w_hbm[k].at[l, pl.ds(r, m)], w_f32[k].at[l, pl.ds(r, m)],
                sems.at[_SEM0["w_load"] + l * _N_WP + j])

        def cast_piece(l, j):
            k, r, m = _W_PIECES[j]
            w_own[k][l, pl.ds(r, m), :] = w_f32[k][l, pl.ds(r, m), :].astype(_BF16)

        def send_piece(l, j):
            k, r, m = _W_PIECES[j]
            remote(w_own[k].at[l, pl.ds(r, m)], w_nbr[k].at[l, pl.ds(r, m)],
                   tx, sems.at[_SEM0["w"] + 2 * l + k], y_nbr).start()

        def swap_pieces(l, pieces):
            for j in pieces:
                load_piece(l, j).wait()
                cast_piece(l, j)
                send_piece(l, j)

        def swap_first_win(l, notify, n_signals, start_next_loads):
            load_piece(l, 0).start()
            load_piece(l, 1).start()
            for dev in notify:
                signal(barrier, dev)
            load_piece(l, 0).wait()
            load_piece(l, 2).start()
            cast_piece(l, 0)
            pl.semaphore_wait(barrier, n_signals)
            send_piece(l, 0)
            swap_pieces(l, [1])
            load_piece(l, 2).wait()
            start_next_loads()
            cast_piece(l, 2)
            send_piece(l, 2)

        def weight_swap(l, k):
            return remote(w_own[k].at[l], w_nbr[k].at[l],
                          tx, sems.at[_SEM0["w"] + 2 * l + k], y_nbr)

        def l2_copy(s, k):
            return remote((w_own, w_nbr)[s][k].at[0], w_l2[k].at[s],
                          tx, sems.at[_SEM0["l2"] + k], x_nbr)

        def partial_copy(i):
            return remote(p_send.at[_chunk(i)], p_recv.at[_chunk(i)], tx,
                          sems.at[_SEM0["partial"] + i], y_nbr)

        def act_copy(i, r=0, m=_C):
            sl = _rows(i * _C + r, m)
            return remote(a_send.at[sl], a_recv.at[sl], last_tx,
                          sems.at[_SEM1["act"] + i], x_nbr)

        def twin_copy(i):
            return remote(a_send.at[_chunk(i)], p_recv.at[_chunk(i)], tx,
                          sems.at[_SEM1["twin"] + i], y_nbr)

        def drained_copy(j):
            return remote(o_send.at[_chunk(j)], o_recv.at[_chunk(j)], last_tx,
                          sems.at[_SEM1["drain"] + list(_DRAIN.values()).index(j)], y_nbr)

        def first_hop(j):
            return remote(o_send.at[_chunk(j)], o_send.at[_chunk(j)], last_tx,
                          sems.at[_SEM0["detour"] + detours.index(j)], x_nbr)

        @pl.when(mx == 0)
        def stage0():
            def x_load(j, m=_L0_ROWS):
                r = j * _L0_ROWS
                return pltpu.make_async_copy(
                    x_hbm.at[0, _rows((oth0 + r) % _ROWS, m)], x_buf.at[_rows(r, m)],
                    sems.at[_SEM0["x_load"] + j])

            def start_layer0_loads():
                for j in range(_N_WP):
                    load_piece(0, j).start()
                x_load(0).start()

            def layer0(sl):
                return _half_layer(x_buf[sl, :].astype(_BF16), wi_own.at[0], wo_own.at[0])

            swap_first_win(1, (y_nbr, x_nbr), 1, start_layer0_loads)
            for j in range(_N_WP):
                load_piece(0, j).wait()
                cast_piece(0, j)
            x_load(1).start()
            for j in range(_N_WIN, _N_WP):
                load_piece(1, j).start()

            n_oth = _HALF // _L0_ROWS

            def layer0_other(j):
                x_load(j).wait()
                x_load(j + 2).start()
                sl = _rows(j * _L0_ROWS, _L0_ROWS)
                p_send[sl, :] = layer0(sl).astype(_BF16)
                pl.when(j == 0)(lambda: swap_pieces(1, range(_N_WIN, _N_WP)))

            _loop(0, n_oth, layer0_other)

            x_load(_N_L0, _N_GAP * _C).start()
            per_block = _N // (_N_L0 - n_oth)
            for j in range(n_oth, _N_L0):
                x_load(j).wait()
                for i in range((j - n_oth) * per_block, (j - n_oth + 1) * per_block):
                    partial_copy(i).start()
                acc[_rows(j * _L0_ROWS - _HALF, _L0_ROWS), :] = layer0(
                    _rows(j * _L0_ROWS, _L0_ROWS))

            out_ref[...] = jnp.zeros(out_ref.shape, _F32)

            x_load(_N_L0, _N_GAP * _C).wait()
            pl.semaphore_wait(x_ready, 1)
            for k in range(2):
                weight_swap(1, k).wait_recv()

            def stream(lo, hi, l2_rows, i):
                partial_copy(i).wait_recv()
                a = (acc[_chunk(i), :] + p_recv[_chunk(i), :].astype(_F32)).astype(_BF16)
                a = full_layer(a, 1).astype(_BF16)
                plain = _C - l2_rows
                a_send[_rows(i * _C, plain), :] = a[:plain]
                act_copy(i, 0, plain).start()
                if l2_rows:
                    if lo == _L2_PLAN[1][0]:
                        for k in range(2):
                            remote(w_l2[k], w_l2[k], tx, sems.at[_SEM0["l2"] + k],
                                   x_nbr).wait_recv()
                    a = (_half_layer(a[plain:], wi_l2.at[0], wo_l2.at[0])
                         + _half_layer(a[plain:], wi_l2.at[1], wo_l2.at[1]))
                    a_send[_rows(i * _C + plain, l2_rows), :] = a.astype(_BF16)
                    act_copy(i, plain, l2_rows).start()
                if hi <= _N_GAP:
                    gap = _N - _N_GAP + i
                    acc[_chunk(gap), :] = layer0(_chunk(_N + gap))
                for j, at in _DETOUR.items():
                    if lo <= at < hi:
                        @pl.when(i == at)
                        def _():
                            first_hop(j).wait_recv()
                            second_hop(end_sems, j).start()

            for lo, hi, l2_rows in _L2_PLAN:
                _loop(lo, hi, functools.partial(stream, lo, hi, l2_rows))

            for k in range(2):
                weight_swap(1, k).wait_send()
            remote(p_send, p_recv, tx, sems.at[_SEM0["partial"]], y_nbr).wait_send()

        @pl.when(mx == 1)
        def stage1():
            def start_other_loads():
                for j in range(_N_WIN, _N_WP):
                    load_piece(0, j).start()
                for j in range(_N_WP):
                    load_piece(1, j).start()

            swap_first_win(0, (y_nbr,), 2, start_other_loads)
            signal(x_ready, x_nbr)
            l2_copy(0, 0).start()
            swap_pieces(0, range(_N_WIN, _N_WP))
            l2_copy(0, 1).start()
            swap_pieces(1, range(_N_WP))
            for k in range(2):
                weight_swap(0, k).wait_recv()
                l2_copy(1, k).start()

            def layer2(i, l2_rows):
                act_copy(i).wait_recv()
                plain = _C - l2_rows
                a = full_layer(a_recv[_rows(i * _C, plain), :], 0).astype(_BF16)
                if l2_rows:
                    a = jnp.concatenate([a, a_recv[_rows(i * _C + plain, l2_rows), :]])
                return a

            def early(twin, i):
                a = layer2(i, 0)
                if twin:
                    a_send[_chunk(i), :] = a
                    twin_copy(i).start()
                acc[_chunk(i), :] = _half_layer(a, wi_own.at[1], wo_own.at[1])
                if not twin:
                    h_buf[_chunk(i - _TWIN), :] = _hidden(a, wi_nbr.at[1])

            def emit(i, out):
                out = out.astype(_BF16)
                o_send[_chunk(i), :] = out
                out_ref[0, _rows(own0 + i * _C), :] = out.astype(_F32)
                if i in _DRAIN:
                    write_received(_DRAIN[i])
                if i in _DETOUR:
                    first_hop(i).start()
                elif i in _TAIL:
                    tail_copy(end_sems, i).start()
                else:
                    drained_copy(i).start()

            _loop(0, _TWIN, functools.partial(early, True))
            weight_swap(1, 0).wait_recv()
            _loop(_TWIN, _EARLY, functools.partial(early, False))
            weight_swap(1, 1).wait_recv()
            for i in range(_TWIN, _EARLY, _EARLY_BATCH):
                out = acc[_chunk(i, _EARLY_BATCH), :] + jnp.dot(
                    h_buf[_chunk(i - _TWIN, _EARLY_BATCH), :], wo_nbr[1],
                    preferred_element_type=_F32)
                for b in range(_EARLY_BATCH):
                    emit(i + b, out[b * _C:(b + 1) * _C])
            for lo, hi, l2_rows in _L2_PLAN:
                for i in range(max(lo, _EARLY), hi):
                    if i in _DRAIN:
                        drained_copy(_DRAIN[i]).wait_recv()
                    emit(i, full_layer(layer2(i, l2_rows), 1))

            for s in range(2):
                for k in range(2):
                    weight_swap(s, k).wait_send()
                    l2_copy(s, k).wait_send()
            for i in range(_TWIN):
                twin_copy(i).wait()

    def end_phase(end_sems):
        pl.run_scoped(functools.partial(main_phase, end_sems),
                      pltpu.SemaphoreType.DMA((max(_N_SEM0, _N_SEM1),)),
                      pltpu.SemaphoreType.REGULAR)

        @pl.when(mx == 0)
        def stage0():
            for j in detours:
                second_hop(end_sems, j).wait_recv()
                third_hop(end_sems, j).start()

        @pl.when(mx == 1)
        def stage1():
            for j in _TAIL[:_TAIL_ARRIVED]:
                tail_copy(end_sems, j).wait_recv()
            sl = _chunk(0, _TWIN)
            own = acc[sl, :] + _half_layer(a_send[sl, :], wi_nbr.at[1], wo_nbr.at[1])
            for row0, out in ((own0, own), (oth0, full_layer(p_recv[sl, :], 1))):
                out_ref[0, _rows(row0, _TWIN * _C), :] = out.astype(_BF16).astype(_F32)
            for j in _TAIL[:_TAIL_ARRIVED]:
                write_received(j)
            for j in _TAIL[_TAIL_ARRIVED:-1]:
                tail_copy(end_sems, j).wait_recv()
                write_received(j)

    pl.run_scoped(end_phase, pltpu.SemaphoreType.DMA((len(_TAIL) - 1,)))

    def wait_sent(src):
        remote(src, src, last_tx, last_rx, y_nbr).wait_send()

    @pl.when(mx == 0)
    def finish0():
        wait_sent(a_send)
        for j in detours:
            wait_sent(o_send.at[_chunk(j)])
            wait_sent(o_recv.at[_chunk(j)])

    @pl.when(mx == 1)
    def finish1():
        wait_sent(o_send.at[_chunk(_TWIN, _N - _TWIN)])
        tail_copy(None, _TAIL[-1]).wait_recv()
        write_received(_TAIL[-1])


def pallas_dist_pipemlp_pp2tp2_xy_b4096_d256_h512_kernel(
    x_padded: jax.Array,
    Win: jax.Array,
    Wout: jax.Array,
):
    assert x_padded.shape == (1, _ROWS, _D)
    assert Win.shape == (2, _D, _HID) and Wout.shape == (2, _HID, _D)
    hbm = pl.BlockSpec(memory_space=pltpu.HBM)
    return pl.pallas_call(
        _kernel,
        out_shape=pltpu.VMEM(x_padded.shape, x_padded.dtype),
        in_specs=[hbm, hbm, hbm],
        out_specs=pl.BlockSpec(memory_space=pltpu.VMEM),
        scratch_shapes=[
            pltpu.VMEM(Win.shape, _F32), pltpu.VMEM(Wout.shape, _F32),
            *[pltpu.VMEM(w.shape, _BF16) for _ in range(3) for w in (Win, Wout)],
            pltpu.VMEM((_ROWS, _D), _F32), pltpu.VMEM((_HALF, _D), _F32),
            pltpu.VMEM(((_EARLY - _TWIN) * _C, _HID), _BF16),
            *[pltpu.VMEM((_HALF, _D), _BF16) for _ in range(6)],
            pltpu.SemaphoreType.DMA, pltpu.SemaphoreType.DMA,
        ],
        compiler_params=pltpu.CompilerParams(
            collective_id=0, vmem_limit_bytes=48 * 1024 * 1024),
    )(x_padded, Win, Wout)
```

```python
import functools

import jax
import jax.numpy as jnp
from jax import lax
from jax.experimental import pallas as pl
from jax.experimental.pallas import tpu as pltpu

_BF16 = jnp.bfloat16
_F32 = jnp.float32

_ROWS, _D, _HID = 4096, 256, 512
_HALF = _ROWS // 2
_C = 128
_N = _HALF // _C
_P = _C // 2

_L2_ON_X0 = (8, 9, 11, 12, 14, 15)
_TWIN, _EARLY = 2, 6
_EARLY_BATCH = 2
_DETOUR = {6: 12, 8: 14, 10: 15}
_DRAIN = {9: 2, 10: 3, 11: 4, 12: 5, 13: 7, 14: 9}
_TAIL = (11, 12, 6, 13, 8, 14, 10, 15)
_TAIL_ARRIVED = 3
assert sorted((*range(_TWIN), *_DRAIN.values(), *_TAIL)) == list(range(_N))
assert set(_DETOUR) <= set(_TAIL[:-1])

_W_PIECES = ((0, 0, 16), (0, 16, 48), (0, 64, 64), (0, 128, 128), (1, 0, 512))
_N_WP, _N_WIN = len(_W_PIECES), 4
_L0_ROWS = 512
_N_GAP, _GAP_ROWS = 8, 64
_N_L0 = (_ROWS - _N_GAP * _GAP_ROWS) // _L0_ROWS
assert _N_L0 * _L0_ROWS + _N_GAP * _GAP_ROWS == _ROWS
assert _HALF - _N_GAP * _GAP_ROWS >= _N_GAP * _C


def _layout(*groups):
    base, at = {}, 0
    for name, count in groups:
        base[name] = at
        at += count
    return base, at


_BOTH = (("tx", 1), ("w_load", 2 * _N_WP), ("w", 4))
_SEM0, _N_SEM0 = _layout(*_BOTH, ("x_load", _N_L0 + 1), ("partial", 2 * _N), ("l2", 2),
                         ("detour", len(_DETOUR)))
_SEM1, _N_SEM1 = _layout(*_BOTH, ("act", _N), ("twin", _TWIN), ("drain", len(_DRAIN)))


def _rows(r, m=_C):
    return pl.ds(r if isinstance(r, int) else pl.multiple_of(r, 16), m)


def _chunk(i, count=1):
    return _rows(i * _C, count * _C)


def _loop(lo, hi, body):
    if hi - lo == 1:
        body(lo)
    else:
        def step(i, carry):
            body(i)
            return carry
        lax.fori_loop(lo, hi, step, 0)


def _hidden(a, wi):
    h = jnp.dot(a, wi[...], preferred_element_type=_F32)
    return jnp.maximum(h, 0.0).astype(_BF16)


def _half_layer(a, wi, wo):
    return jnp.dot(_hidden(a, wi), wo[...], preferred_element_type=_F32)


def _kernel(
    x_hbm, win_hbm, wout_hbm, out_ref,
    wi_f32, wo_f32, wi_own, wo_own, wi_nbr, wo_nbr, wi_l2, wo_l2,
    x_buf, acc, h_buf, p_send, p_recv, a_send, a_recv, o_send, o_recv, last_tx, last_rx,
):
    mx, my = lax.axis_index("x"), lax.axis_index("y")
    y_nbr, x_nbr = (mx, 1 - my), (1 - mx, my)
    own0, oth0 = my * _HALF, (1 - my) * _HALF
    w_hbm, w_f32 = (win_hbm, wout_hbm), (wi_f32, wo_f32)
    w_own, w_nbr, w_l2 = (wi_own, wo_own), (wi_nbr, wo_nbr), (wi_l2, wo_l2)
    detours = list(_DETOUR)

    def remote(src, dst, tx, rx, dev):
        return pltpu.make_async_remote_copy(
            src, dst, tx, rx, device_id=dev, device_id_type=pl.DeviceIdType.MESH)

    def signal(sem, dev):
        pl.semaphore_signal(sem, inc=1, device_id=dev, device_id_type=pl.DeviceIdType.MESH)

    def full_layer(a, l):
        return (_half_layer(a, wi_own.at[l], wo_own.at[l])
                + _half_layer(a, wi_nbr.at[l], wo_nbr.at[l]))

    def write_received(j):
        out_ref[0, _rows(oth0 + j * _C), :] = o_recv[_chunk(j), :].astype(_F32)

    def tail_sem(end_sems, j):
        return last_rx if j == _TAIL[-1] else end_sems.at[_TAIL.index(j)]

    def tail_copy(end_sems, j):
        return remote(o_send.at[_chunk(j)], o_recv.at[_chunk(j)], last_tx,
                      tail_sem(end_sems, j), y_nbr)

    def second_hop(end_sems, j):
        return remote(o_send.at[_chunk(j)], o_recv.at[_chunk(j)], last_tx,
                      end_sems.at[detours.index(j)], y_nbr)

    def third_hop(end_sems, j):
        return remote(o_recv.at[_chunk(j)], o_recv.at[_chunk(j)], last_tx,
                      tail_sem(end_sems, j), x_nbr)

    def main_phase(end_sems, sems, x_ready):
        barrier = pltpu.get_barrier_semaphore()
        tx = sems.at[_SEM0["tx"]]

        def load_piece(l, j):
            k, r, m = _W_PIECES[j]
            return pltpu.make_async_copy(
                w_hbm[k].at[l, pl.ds(r, m)], w_f32[k].at[l, pl.ds(r, m)],
                sems.at[_SEM0["w_load"] + l * _N_WP + j])

        def cast_piece(l, j):
            k, r, m = _W_PIECES[j]
            w_own[k][l, pl.ds(r, m), :] = w_f32[k][l, pl.ds(r, m), :].astype(_BF16)

        def send_piece(l, j):
            k, r, m = _W_PIECES[j]
            remote(w_own[k].at[l, pl.ds(r, m)], w_nbr[k].at[l, pl.ds(r, m)],
                   tx, sems.at[_SEM0["w"] + 2 * l + k], y_nbr).start()

        def swap_pieces(l, pieces):
            for j in pieces:
                load_piece(l, j).wait()
                cast_piece(l, j)
                send_piece(l, j)

        def swap_first_win(l, notify, n_signals, start_next_loads):
            load_piece(l, 0).start()
            load_piece(l, 1).start()
            for dev in notify:
                signal(barrier, dev)
            load_piece(l, 0).wait()
            load_piece(l, 2).start()
            cast_piece(l, 0)
            pl.semaphore_wait(barrier, n_signals)
            send_piece(l, 0)
            swap_pieces(l, [1])
            load_piece(l, 3).start()
            load_piece(l, 2).wait()
            start_next_loads()
            cast_piece(l, 2)
            send_piece(l, 2)
            swap_pieces(l, [3])

        def weight_swap(l, k):
            return remote(w_own[k].at[l], w_nbr[k].at[l],
                          tx, sems.at[_SEM0["w"] + 2 * l + k], y_nbr)

        def l2_copy(s, k):
            return remote((w_own, w_nbr)[s][k].at[0], w_l2[k].at[s],
                          tx, sems.at[_SEM0["l2"] + k], x_nbr)

        def partial_copy(q):
            sl = _rows(q * _P, _P)
            return remote(p_send.at[sl], p_recv.at[sl], tx,
                          sems.at[_SEM0["partial"] + q], y_nbr)

        def act_copy(i, sl):
            return remote(a_send.at[sl], a_recv.at[sl], last_tx,
                          sems.at[_SEM1["act"] + i], x_nbr)

        def twin_copy(i):
            return remote(a_send.at[_chunk(i)], p_recv.at[_chunk(i)], tx,
                          sems.at[_SEM1["twin"] + i], y_nbr)

        def drained_copy(j):
            return remote(o_send.at[_chunk(j)], o_recv.at[_chunk(j)], last_tx,
                          sems.at[_SEM1["drain"] + list(_DRAIN.values()).index(j)], y_nbr)

        def first_hop(j):
            return remote(o_send.at[_chunk(j)], o_send.at[_chunk(j)], last_tx,
                          sems.at[_SEM0["detour"] + detours.index(j)], x_nbr)

        @pl.when(mx == 0)
        def stage0():
            def x_load(j, m=_L0_ROWS):
                r = j * _L0_ROWS
                return pltpu.make_async_copy(
                    x_hbm.at[0, _rows((oth0 + r) % _ROWS, m)], x_buf.at[_rows(r, m)],
                    sems.at[_SEM0["x_load"] + j])

            def start_layer0_loads():
                for j in range(_N_WP):
                    load_piece(0, j).start()
                x_load(0).start()

            def layer0(sl):
                return _half_layer(x_buf[sl, :].astype(_BF16), wi_own.at[0], wo_own.at[0])

            swap_first_win(1, (y_nbr, x_nbr), 1, start_layer0_loads)
            for j in range(_N_WP):
                load_piece(0, j).wait()
                cast_piece(0, j)
            x_load(1).start()
            for j in range(_N_WIN, _N_WP):
                load_piece(1, j).start()

            n_oth = _HALF // _L0_ROWS

            def layer0_other(j):
                x_load(j).wait()
                x_load(j + 2).start()
                sl = _rows(j * _L0_ROWS, _L0_ROWS)
                p_send[sl, :] = layer0(sl).astype(_BF16)
                pl.when(j == 0)(lambda: swap_pieces(1, range(_N_WIN, _N_WP)))

            _loop(0, n_oth, layer0_other)

            x_load(_N_L0, _N_GAP * _GAP_ROWS).start()
            n_own = _N_L0 - n_oth
            for j in range(n_oth, _N_L0):
                x_load(j).wait()
                if j + 2 < _N_L0:
                    x_load(j + 2).start()
                b = j - n_oth
                for q in range(b * 2 * _N // n_own, (b + 1) * 2 * _N // n_own):
                    partial_copy(q).start()
                acc[_rows(j * _L0_ROWS - _HALF, _L0_ROWS), :] = layer0(
                    _rows(j * _L0_ROWS, _L0_ROWS))

            x_load(_N_L0, _N_GAP * _GAP_ROWS).wait()
            pl.semaphore_wait(x_ready, 1)
            for k in range(2):
                weight_swap(1, k).wait_recv()

            def stream(lo, hi, i):
                def part(p):
                    sl = _rows(i * _C + p * _P, _P)
                    partial_copy(2 * i + p).wait_recv()
                    a = (acc[sl, :] + p_recv[sl, :].astype(_F32)).astype(_BF16)
                    a = full_layer(a, 1).astype(_BF16)
                    if p == 1 and lo in _L2_ON_X0:
                        if lo == _L2_ON_X0[0]:
                            for k in range(2):
                                remote(w_l2[k], w_l2[k], tx, sems.at[_SEM0["l2"] + k],
                                       x_nbr).wait_recv()
                        a = (_half_layer(a, wi_l2.at[0], wo_l2.at[0])
                             + _half_layer(a, wi_l2.at[1], wo_l2.at[1])).astype(_BF16)
                    a_send[sl, :] = a
                    act_copy(i, sl).start()

                part(0)

                @pl.when(my >= 0)
                def _():
                    part(1)
                    if hi <= _N_GAP:
                        r = _HALF - (_N_GAP - i) * _GAP_ROWS
                        acc[_rows(r, _GAP_ROWS), :] = layer0(_rows(_HALF + r, _GAP_ROWS))

                for j, at in _DETOUR.items():
                    if lo <= at < hi:
                        @pl.when(i == at)
                        def _():
                            first_hop(j).wait_recv()
                            second_hop(end_sems, j).start()

            def kind(i):
                return i < _N_GAP, i in _L2_ON_X0, i == _L2_ON_X0[0]

            starts = [i for i in range(_N) if i == 0 or kind(i) != kind(i - 1)]
            for lo, hi in zip(starts, starts[1:] + [_N]):
                _loop(lo, hi, functools.partial(stream, lo, hi))

            for k in range(2):
                weight_swap(1, k).wait_send()
            remote(p_send, p_recv, tx, sems.at[_SEM0["partial"]], y_nbr).wait_send()

        @pl.when(mx == 1)
        def stage1():
            def start_other_loads():
                for j in range(_N_WIN, _N_WP):
                    load_piece(0, j).start()
                for j in range(_N_WP):
                    load_piece(1, j).start()

            swap_first_win(0, (y_nbr,), 2, start_other_loads)
            signal(x_ready, x_nbr)
            l2_copy(0, 0).start()
            swap_pieces(0, range(_N_WIN, _N_WP))
            l2_copy(0, 1).start()
            swap_pieces(1, range(_N_WP))
            for k in range(2):
                weight_swap(0, k).wait_recv()
                l2_copy(1, k).start()

            def layer2(i, l2_rows):
                act_copy(i, _chunk(i)).wait_recv()
                plain = _C - l2_rows
                a = full_layer(a_recv[_rows(i * _C, plain), :], 0).astype(_BF16)
                if l2_rows:
                    a = jnp.concatenate([a, a_recv[_rows(i * _C + plain, l2_rows), :]])
                return a

            def early(twin, i):
                a = layer2(i, 0)
                if twin:
                    a_send[_chunk(i), :] = a
                    twin_copy(i).start()
                acc[_chunk(i), :] = _half_layer(a, wi_own.at[1], wo_own.at[1])
                if not twin:
                    h_buf[_chunk(i - _TWIN), :] = _hidden(a, wi_nbr.at[1])

            def emit(i, out):
                out = out.astype(_BF16)
                o_send[_chunk(i), :] = out
                out_ref[0, _rows(own0 + i * _C), :] = out.astype(_F32)
                if i in _DRAIN:
                    write_received(_DRAIN[i])
                if i in _DETOUR:
                    first_hop(i).start()
                elif i in _TAIL:
                    tail_copy(end_sems, i).start()
                else:
                    drained_copy(i).start()

            _loop(0, _TWIN, functools.partial(early, True))
            weight_swap(1, 0).wait_recv()
            _loop(_TWIN, _EARLY, functools.partial(early, False))
            weight_swap(1, 1).wait_recv()
            for i in range(_TWIN, _EARLY, _EARLY_BATCH):
                out = acc[_chunk(i, _EARLY_BATCH), :] + jnp.dot(
                    h_buf[_chunk(i - _TWIN, _EARLY_BATCH), :], wo_nbr[1],
                    preferred_element_type=_F32)
                for b in range(_EARLY_BATCH):
                    emit(i + b, out[b * _C:(b + 1) * _C])
            for i in range(_EARLY, _N):
                if i in _DRAIN:
                    drained_copy(_DRAIN[i]).wait_recv()
                emit(i, full_layer(layer2(i, _P if i in _L2_ON_X0 else 0), 1))

            for s in range(2):
                for k in range(2):
                    weight_swap(s, k).wait_send()
                    l2_copy(s, k).wait_send()
            for i in range(_TWIN):
                twin_copy(i).wait()

    def end_phase(end_sems):
        pl.run_scoped(functools.partial(main_phase, end_sems),
                      pltpu.SemaphoreType.DMA((max(_N_SEM0, _N_SEM1),)),
                      pltpu.SemaphoreType.REGULAR)

        @pl.when(mx == 0)
        def stage0():
            for j in detours:
                second_hop(end_sems, j).wait_recv()
                third_hop(end_sems, j).start()
                if j == detours[0]:
                    def zero(i):
                        out_ref[0, _chunk(4 * i, 4), :] = jnp.zeros((4 * _C, _D), _F32)

                    _loop(0, _ROWS // (4 * _C), zero)

        @pl.when(mx == 1)
        def stage1():
            for j in _TAIL[:_TAIL_ARRIVED]:
                tail_copy(end_sems, j).wait_recv()
            sl = _chunk(0, _TWIN)
            own = acc[sl, :] + _half_layer(a_send[sl, :], wi_nbr.at[1], wo_nbr.at[1])
            for row0, out in ((own0, own), (oth0, full_layer(p_recv[sl, :], 1))):
                out_ref[0, _rows(row0, _TWIN * _C), :] = out.astype(_BF16).astype(_F32)
            for j in _TAIL[:_TAIL_ARRIVED]:
                write_received(j)
            for j in _TAIL[_TAIL_ARRIVED:-1]:
                tail_copy(end_sems, j).wait_recv()
                write_received(j)

    pl.run_scoped(end_phase, pltpu.SemaphoreType.DMA((len(_TAIL) - 1,)))

    def wait_sent(src):
        remote(src, src, last_tx, last_rx, y_nbr).wait_send()

    @pl.when(mx == 0)
    def finish0():
        wait_sent(a_send)
        for j in detours:
            wait_sent(o_send.at[_chunk(j)])
            wait_sent(o_recv.at[_chunk(j)])

    @pl.when(mx == 1)
    def finish1():
        wait_sent(o_send.at[_chunk(_TWIN, _N - _TWIN)])
        tail_copy(None, _TAIL[-1]).wait_recv()
        write_received(_TAIL[-1])


def pallas_dist_pipemlp_pp2tp2_xy_b4096_d256_h512_kernel(
    x_padded: jax.Array,
    Win: jax.Array,
    Wout: jax.Array,
):
    assert x_padded.shape == (1, _ROWS, _D)
    assert Win.shape == (2, _D, _HID) and Wout.shape == (2, _HID, _D)
    hbm = pl.BlockSpec(memory_space=pltpu.HBM)
    return pl.pallas_call(
        _kernel,
        out_shape=pltpu.VMEM(x_padded.shape, x_padded.dtype),
        in_specs=[hbm, hbm, hbm],
        out_specs=pl.BlockSpec(memory_space=pltpu.VMEM),
        scratch_shapes=[
            pltpu.VMEM(Win.shape, _F32), pltpu.VMEM(Wout.shape, _F32),
            *[pltpu.VMEM(w.shape, _BF16) for _ in range(3) for w in (Win, Wout)],
            pltpu.VMEM((_ROWS, _D), _F32), pltpu.VMEM((_HALF, _D), _F32),
            pltpu.VMEM(((_EARLY - _TWIN) * _C, _HID), _BF16),
            *[pltpu.VMEM((_HALF, _D), _BF16) for _ in range(6)],
            pltpu.SemaphoreType.DMA, pltpu.SemaphoreType.DMA,
        ],
        compiler_params=pltpu.CompilerParams(
            collective_id=0, vmem_limit_bytes=48 * 1024 * 1024),
    )(x_padded, Win, Wout)
```
